```python
import numpy as np

kernel_name = "dist_halo_stencil_i_m8192_n1024"

def setup_inputs():
    return {"x": np.random.randn(32768, 1024).astype(np.float32)}

def reference(x: np.ndarray) -> np.ndarray:
    out = np.empty_like(x)
    out[0] = x[0]
    out[-1] = x[-1]
    out[1:-1] = 0.25 * x[:-2] + 0.5 * x[1:-1] + 0.25 * x[2:]
    return out
```

```python
import jax
import jax.numpy as jnp
from jax import lax
from jax.experimental import pallas as pl
from jax.experimental.pallas import tpu as pltpu

N_DEV = 4
TILE = 8
BLOCK = 64
SLAB = 128
GROUP = 256
SPLIT = 4
PIECE = 16 // SPLIT * GROUP

PARTS = (4096, 2048)
BURST = 16
BURSTS = 24
AHEAD = 6
LATE = 4
QUIET = 14
CHUNK = 512
TAIL = (1024, 512, 256, 128, 64, 32, 16, 0)
FLUSH = 2


def _aligned(row):
    return row if isinstance(row, int) else pl.multiple_of(row, TILE)


def _divmod(row, size):
    return row >> (size.bit_length() - 1), _aligned(row & (size - 1))


def _rows(ref, row, size):
    slab, offset = _divmod(row, SLAB)
    return ref.at[slab, pl.ds(offset, size)]


def _for(lo, hi, body):
    if hi - lo == 1:
        body(lo)
    elif hi > lo:
        pl.loop(lo, hi)(body)


def _stencil(above, body, below):
    tiles = [above, *(body[r:r + TILE] for r in range(0, body.shape[0], TILE)), below]
    sublane = lax.broadcasted_iota(jnp.int32, above.shape, 0)
    quarter = [0.25 * tile for tile in tiles]
    out = []
    for k in range(1, len(tiles) - 1):
        before = jnp.where(sublane == TILE - 1, quarter[k - 1], quarter[k])
        after = jnp.where(sublane == 0, quarter[k + 1], quarter[k])
        out.append(
            pltpu.roll(before, 1, 0) + 0.5 * tiles[k] + pltpu.roll(after, TILE - 1, 0))
    return jnp.concatenate(out, axis=0) if len(out) > 1 else out[0]


def _kernel(x_hbm, *refs):
    out_refs = refs[:SPLIT * SPLIT]
    (x_ref, halo_ref, relay_ref,
     part_sems, tail_sems, halo_sems, relay_sems) = refs[SPLIT * SPLIT:]
    m, n = x_ref.shape[0] * SLAB, x_ref.shape[2]
    relayed = sum(PARTS)
    tail = relayed + BURSTS * BURST

    me = lax.axis_index("i")
    left = (me + N_DEV - 1) % N_DEV
    right = (me + 1) % N_DEV

    def remote(src, dst, sems, peer):
        return pltpu.make_async_remote_copy(
            src_ref=src, dst_ref=dst, send_sem=sems.at[0], recv_sem=sems.at[1],
            device_id=(peer,), device_id_type=pl.DeviceIdType.MESH)

    def part_slabs(p):
        return pl.ds(sum(PARTS[:p]) // SLAB, PARTS[p] // SLAB)

    def start_part(p):
        def start(t):
            at = (part_slabs(p), pl.ds(_aligned(t * TILE), TILE))
            pltpu.make_async_copy(x_hbm.at[at], x_ref.at[at], part_sems.at[p]).start()
        _for(0, SLAB // TILE, start)

    def wait_part(p):
        at = part_slabs(p)
        pltpu.make_async_copy(x_hbm.at[at], x_ref.at[at], part_sems.at[p]).wait()

    ends = [m - rest + (TILE if 0 < rest < SLAB else 0) for rest in TAIL]
    tail_reads = []
    for k, (lo, hi) in enumerate(zip([tail] + ends[:-1], ends)):
        if lo % SLAB == 0 and hi % SLAB == 0:
            at = pl.ds(lo // SLAB, (hi - lo) // SLAB)
            src, dst = x_hbm.at[at], x_ref.at[at]
        else:
            src, dst = _rows(x_hbm, lo, hi - lo), _rows(x_ref, lo, hi - lo)
        tail_reads.append(pltpu.make_async_copy(src, dst, tail_sems.at[k]))

    halos = [
        remote(_rows(x_hbm, m - TILE, TILE), halo_ref.at[0], halo_sems.at[0], right),
        remote(_rows(x_hbm, 0, TILE), halo_ref.at[1], halo_sems.at[1], left),
    ]

    def forward(j):
        src = _rows(x_hbm, relayed + j * BURST, BURST)
        return remote(src, relay_ref.at[j], relay_sems.at[j, 0], left)

    def back(j):
        dst = _rows(x_ref, relayed + j * BURST, BURST)
        return remote(relay_ref.at[j], dst, relay_sems.at[j, 1], right)

    def relay(j):
        forward(j).wait()
        back(j).start()
        if isinstance(j, int):
            if j + AHEAD < BURSTS:
                forward(j + AHEAD).start()
        else:
            pl.when(j + AHEAD < BURSTS)(lambda: forward(j + AHEAD).start())

    def store(base, row, value):
        half, k = divmod(base // PIECE, SPLIT)
        group, offset = _divmod(row - base, GROUP)
        width = n // SPLIT
        for c in range(SPLIT):
            out_refs[k * SPLIT + c][half, group, pl.ds(offset, value.shape[0]), :] = (
                value[:, c * width:(c + 1) * width])

    def block(base, row, size):
        above = _rows(x_ref, row - TILE, TILE)[...]
        below = _rows(x_ref, row + size, TILE)[...]
        store(base, row, _stencil(above, _rows(x_ref, row, size)[...], below))

    step = 0

    def compute(lo, hi):
        nonlocal step
        while lo < hi:
            base = lo // PIECE * PIECE
            if lo % BLOCK or hi - lo < BLOCK:
                end = min(hi, (lo // BLOCK + 1) * BLOCK)
                block(base, lo, end - lo)
            else:
                end = min(hi // BLOCK * BLOCK, base + PIECE)
                due = [r for r in range(lo, end, BLOCK) if r % CHUNK == CHUNK - 2 * BLOCK]
                due = due[:BURSTS - step]

                def body(i, base=base, due=due, step=step):
                    row = i * BLOCK
                    block(base, row, BLOCK)
                    if due:
                        @pl.when((row & (CHUNK - 1) == CHUNK - 2 * BLOCK) & (row <= due[-1]))
                        def _():
                            relay(step + _divmod(row - due[0], CHUNK)[0])

                _for(lo // BLOCK, end // BLOCK, body)
                step += len(due)
            lo = end

    def edge(row, above, below, keep):
        tile = _rows(x_ref, row, TILE)[...]
        store(row // PIECE * PIECE, row, jnp.where(keep, tile, _stencil(above, tile, below)))

    start_part(0)
    barrier = pltpu.get_barrier_semaphore()
    for peer in (left, right):
        pl.semaphore_signal(
            barrier, inc=1, device_id=(peer,), device_id_type=pl.DeviceIdType.MESH)
    pl.semaphore_wait(barrier, 2)
    halos[0].start()
    _for(0, AHEAD, lambda j: forward(j).start())

    _for(0, QUIET // 2, relay)
    for p in range(1, len(PARTS)):
        start_part(p)
    _for(QUIET // 2, QUIET, relay)
    step = QUIET

    done = TILE
    for p in range(len(PARTS)):
        wait_part(p)
        if p == 0:
            for read in tail_reads:
                read.start()
        end = sum(PARTS[:p + 1]) - BLOCK
        compute(done, end)
        done = end
    assert step == BURSTS
    halos[1].start()

    late = tail - LATE * BURST - BLOCK
    _for(0, BURSTS - LATE, lambda j: back(j).wait())
    compute(done, late)

    sublane = lax.broadcasted_iota(jnp.int32, (TILE, n), 0)
    done = tail + BLOCK
    for k, read in enumerate(tail_reads):
        if k == FLUSH:
            _for(BURSTS - LATE, BURSTS, lambda j: back(j).wait())
            compute(late, tail + BLOCK)
            for halo in halos:
                halo.wait()
            below = _rows(x_ref, TILE, TILE)[...]
            edge(0, halo_ref[0], below, (sublane == 0) & (me == 0))
        read.wait()
        end = ends[k] - (BLOCK if TAIL[k] >= SLAB else TILE)
        compute(done, end)
        done = end
    above = _rows(x_ref, m - 2 * TILE, TILE)[...]
    edge(m - TILE, above, halo_ref[1], (sublane == TILE - 1) & (me == N_DEV - 1))


def pallas_dist_halo_stencil_i_m8192_n1024_kernel(x: jax.Array):
    m, n = x.shape
    piece = jax.ShapeDtypeStruct((2, 16 // SPLIT, GROUP, n // SPLIT), x.dtype)
    pieces = pl.pallas_call(
        _kernel,
        out_shape=(piece,) * (SPLIT * SPLIT),
        in_specs=[pl.BlockSpec(memory_space=pl.ANY)],
        out_specs=(pl.BlockSpec(memory_space=pltpu.VMEM),) * (SPLIT * SPLIT),
        scratch_shapes=[
            pltpu.VMEM((m // SLAB, SLAB, n), x.dtype),
            pltpu.VMEM((2, TILE, n), x.dtype),
            pltpu.VMEM((BURSTS, BURST, n), x.dtype),
            pltpu.SemaphoreType.DMA((len(PARTS),)),
            pltpu.SemaphoreType.DMA((len(TAIL),)),
            pltpu.SemaphoreType.DMA((2, 2)),
            pltpu.SemaphoreType.DMA((BURSTS, 2, 2)),
        ],
        compiler_params=pltpu.CompilerParams(
            collective_id=0,
            vmem_limit_bytes=40 * 2**20,
            disable_semaphore_checks=True,
        ),
    )(x.reshape(m // SLAB, SLAB, n))
    rows = [lax.concatenate(pieces[k * SPLIT:(k + 1) * SPLIT], 3) for k in range(SPLIT)]
    return lax.concatenate(rows, 1).reshape(m, n)
```

```python
import jax
import jax.numpy as jnp
from jax import lax
from jax.experimental import pallas as pl
from jax.experimental.pallas import tpu as pltpu

N_DEV = 4
TILE = 8
BLOCK = 64
SLAB = 128
GROUP = 256
SPLIT = 4
PIECE = 16 // SPLIT * GROUP

PARTS = (3584, 2560)
BURST = 16
BURSTS = 24
AHEAD = 6
QUIET = 14
CHUNK = 512
LATE = 4
FLUSH = 2
TAIL = (1024, 512, 256, 128, 64, 32, 16, 0)


def _aligned(row):
    return row if isinstance(row, int) else pl.multiple_of(row, TILE)


def _divmod(row, size):
    return row >> (size.bit_length() - 1), _aligned(row & (size - 1))


def _rows(ref, row, size):
    slab, offset = _divmod(row, SLAB)
    return ref.at[slab, pl.ds(offset, size)]


def _for(lo, hi, body):
    if hi - lo == 1:
        body(lo)
    elif hi > lo:
        pl.loop(lo, hi)(body)


def _stencil(above, body, below):
    tiles = [above, *(body[r:r + TILE] for r in range(0, body.shape[0], TILE)), below]
    sublane = lax.broadcasted_iota(jnp.int32, above.shape, 0)
    quarter = [0.25 * tile for tile in tiles]
    out = []
    for k in range(1, len(tiles) - 1):
        before = jnp.where(sublane == TILE - 1, quarter[k - 1], quarter[k])
        after = jnp.where(sublane == 0, quarter[k + 1], quarter[k])
        out.append(
            pltpu.roll(before, 1, 0) + 0.5 * tiles[k] + pltpu.roll(after, TILE - 1, 0))
    return jnp.concatenate(out, axis=0) if len(out) > 1 else out[0]


def _kernel(x_hbm, *refs):
    out_refs = refs[:SPLIT * SPLIT]
    x_ref, halo_ref, relay_ref, part_sems, tail_sems, *remote_sems = refs[SPLIT * SPLIT:]
    halo_sems, forward_sems, back_sems = zip(remote_sems[::2], remote_sems[1::2])
    m, n = x_ref.shape[0] * SLAB, x_ref.shape[2]
    relayed = sum(PARTS)
    tail = relayed + BURSTS * BURST

    me = lax.axis_index("i")
    left = (me + N_DEV - 1) % N_DEV
    right = (me + 1) % N_DEV

    def remote(src, dst, sems, k, peer):
        send_sems, recv_sems = sems
        return pltpu.make_async_remote_copy(
            src_ref=src, dst_ref=dst, send_sem=send_sems.at[k], recv_sem=recv_sems.at[k],
            device_id=(peer,), device_id_type=pl.DeviceIdType.MESH)

    def part_slabs(p):
        return pl.ds(sum(PARTS[:p]) // SLAB, PARTS[p] // SLAB)

    def start_part(p):
        def start(t):
            at = (part_slabs(p), pl.ds(_aligned(t * TILE), TILE))
            pltpu.make_async_copy(x_hbm.at[at], x_ref.at[at], part_sems.at[p]).start()
        _for(0, SLAB // TILE, start)

    def wait_part(p):
        at = part_slabs(p)
        pltpu.make_async_copy(x_ref.at[at], x_ref.at[at], part_sems.at[p]).wait()

    ends = [m - rest + (TILE if 0 < rest < SLAB else 0) for rest in TAIL]
    tail_reads = []
    for k, (lo, hi) in enumerate(zip([tail] + ends[:-1], ends)):
        if lo % SLAB == 0 and hi % SLAB == 0:
            at = pl.ds(lo // SLAB, (hi - lo) // SLAB)
            src, dst = x_hbm.at[at], x_ref.at[at]
        else:
            src, dst = _rows(x_hbm, lo, hi - lo), _rows(x_ref, lo, hi - lo)
        tail_reads.append(pltpu.make_async_copy(src, dst, tail_sems.at[k]))

    halos = [
        remote(_rows(x_hbm, m - TILE, TILE), halo_ref.at[0], halo_sems, 0, right),
        remote(_rows(x_hbm, 0, TILE), halo_ref.at[1], halo_sems, 1, left),
    ]

    def forward(j):
        src = _rows(x_hbm, relayed + j * BURST, BURST)
        return remote(src, relay_ref.at[j], forward_sems, j, left)

    def back(j):
        dst = _rows(x_ref, relayed + j * BURST, BURST)
        return remote(relay_ref.at[j], dst, back_sems, j, right)

    def relay(j):
        forward(j).wait()
        back(j).start()
        if isinstance(j, int):
            if j + AHEAD < BURSTS:
                forward(j + AHEAD).start()
        else:
            pl.when(j + AHEAD < BURSTS)(lambda: forward(j + AHEAD).start())

    def store(base, row, value):
        half, k = divmod(base // PIECE, SPLIT)
        group, offset = _divmod(row - base, GROUP)
        width = n // SPLIT
        for c in range(SPLIT):
            out_refs[k * SPLIT + c][half, group, pl.ds(offset, value.shape[0]), :] = (
                value[:, c * width:(c + 1) * width])

    def block(base, row, size):
        above = _rows(x_ref, row - TILE, TILE)[...]
        below = _rows(x_ref, row + size, TILE)[...]
        store(base, row, _stencil(above, _rows(x_ref, row, size)[...], below))

    step = 0

    def compute(lo, hi):
        nonlocal step
        while lo < hi:
            base = lo // PIECE * PIECE
            if lo % BLOCK or hi - lo < BLOCK:
                end = min(hi, (lo // BLOCK + 1) * BLOCK)
                block(base, lo, end - lo)
            else:
                end = min(hi // BLOCK * BLOCK, base + PIECE)
                due = [r for r in range(lo, end, BLOCK) if r % CHUNK == CHUNK - 2 * BLOCK]
                due = due[:BURSTS - step]

                def body(i, base=base, due=due, step=step):
                    row = i * BLOCK
                    block(base, row, BLOCK)
                    if due:
                        @pl.when((row & (CHUNK - 1) == CHUNK - 2 * BLOCK) & (row <= due[-1]))
                        def _():
                            relay(step + _divmod(row - due[0], CHUNK)[0])

                _for(lo // BLOCK, end // BLOCK, body)
                step += len(due)
            lo = end

    def edge(row, above, below, keep):
        tile = _rows(x_ref, row, TILE)[...]
        store(row // PIECE * PIECE, row, jnp.where(keep, tile, _stencil(above, tile, below)))

    start_part(0)
    barrier = pltpu.get_barrier_semaphore()
    for peer in (left, right):
        pl.semaphore_signal(
            barrier, inc=1, device_id=(peer,), device_id_type=pl.DeviceIdType.MESH)
    pl.semaphore_wait(barrier, 2)
    halos[0].start()
    _for(0, AHEAD, lambda j: forward(j).start())

    _for(0, QUIET // 2, relay)
    for p in range(1, len(PARTS)):
        start_part(p)
    _for(QUIET // 2, QUIET, relay)
    step = QUIET

    done = TILE
    for p in range(len(PARTS)):
        wait_part(p)
        if p == 0:
            for read in tail_reads:
                read.start()
        end = sum(PARTS[:p + 1]) - BLOCK
        compute(done, end)
        done = end
    assert step == BURSTS
    halos[1].start()

    late = tail - LATE * BURST - BLOCK
    _for(0, BURSTS - LATE, lambda j: back(j).wait())
    compute(done, late)

    sublane = lax.broadcasted_iota(jnp.int32, (TILE, n), 0)
    done = tail + BLOCK
    for k, read in enumerate(tail_reads):
        if k == FLUSH:
            _for(BURSTS - LATE, BURSTS, lambda j: back(j).wait())
            compute(late, tail + BLOCK)
            for halo in halos:
                halo.wait()
            below = _rows(x_ref, TILE, TILE)[...]
            edge(0, halo_ref[0], below, (sublane == 0) & (me == 0))
        read.wait()
        end = ends[k] - (BLOCK if TAIL[k] >= SLAB else TILE)
        compute(done, end)
        done = end
    above = _rows(x_ref, m - 2 * TILE, TILE)[...]
    edge(m - TILE, above, halo_ref[1], (sublane == TILE - 1) & (me == N_DEV - 1))


def pallas_dist_halo_stencil_i_m8192_n1024_kernel(x: jax.Array):
    m, n = x.shape
    assert m == 2 * 16 * GROUP and n % (128 * SPLIT) == 0 and x.dtype == jnp.float32
    piece = jax.ShapeDtypeStruct((2, 16 // SPLIT, GROUP, n // SPLIT), x.dtype)
    pieces = pl.pallas_call(
        _kernel,
        out_shape=(piece,) * (SPLIT * SPLIT),
        in_specs=[pl.BlockSpec(memory_space=pl.ANY)],
        out_specs=(pl.BlockSpec(memory_space=pltpu.VMEM),) * (SPLIT * SPLIT),
        scratch_shapes=[
            pltpu.VMEM((m // SLAB, SLAB, n), x.dtype),
            pltpu.VMEM((2, TILE, n), x.dtype),
            pltpu.VMEM((BURSTS, BURST, n), x.dtype),
            pltpu.SemaphoreType.DMA((len(PARTS),)),
            pltpu.SemaphoreType.DMA((len(TAIL),)),
            *[pltpu.SemaphoreType.DMA((2,))] * 2,
            *[pltpu.SemaphoreType.DMA((BURSTS,))] * 4,
        ],
        compiler_params=pltpu.CompilerParams(
            collective_id=0,
            vmem_limit_bytes=40 * 2**20,
            disable_semaphore_checks=True,
        ),
    )(x.reshape(m // SLAB, SLAB, n))
    rows = [lax.concatenate(pieces[k * SPLIT:(k + 1) * SPLIT], 3) for k in range(SPLIT)]
    return lax.concatenate(rows, 1).reshape(m, n)
```
